```python
import numpy as np

kernel_name = "dist_rmsnorm_colshard_i_m768_n512"

def setup_inputs():
    x = np.random.randn(768, 2048).astype(np.float32)
    gamma = np.random.randn(2048).astype(np.float32)
    return {"x": x, "gamma": gamma}

def reference(x: np.ndarray, gamma: np.ndarray) -> np.ndarray:
    eps = 1e-5
    rms = np.sqrt(np.mean(x * x, axis=1, keepdims=True) + eps)
    return gamma * x / rms
```

```python
import jax
import jax.numpy as jnp
from jax import lax
from jax.experimental import pallas as pl
from jax.experimental.pallas import tpu as pltpu

_N_DEV = 4
_EPS = 1e-5
_LANES = 128
_SUBLANES = 8
_TILE = (_SUBLANES, _LANES)
_CHUNKS = (256, 256, 128, 80, 48)
_N_TAIL = 3


def _pack(col):
    sublane = lax.broadcasted_iota(jnp.int32, _TILE, 0)
    lane = lax.broadcasted_iota(jnp.int32, _TILE, 1)

    def merge(lo, hi):
        if hi - lo == _SUBLANES:
            return jnp.broadcast_to(col[lo:hi], _TILE)
        mid = lo + (hi - lo) // (2 * _SUBLANES) * _SUBLANES
        return jnp.where(lane < mid, merge(lo, mid), merge(mid, hi))

    own_row = (lane & (_SUBLANES - 1)) == sublane
    picked = jnp.where(own_row, merge(0, col.shape[0]), 0.0)
    return jnp.sum(picked, axis=0, keepdims=True)


def _unpack(line, rows):
    row = lax.broadcasted_iota(jnp.int32, (rows, _LANES), 0)
    lane = lax.broadcasted_iota(jnp.int32, (rows, _LANES), 1)
    return jnp.sum(jnp.where(row == lane, line, 0.0), axis=1, keepdims=True)


def pallas_dist_rmsnorm_colshard_i_m768_n512_kernel(
    x: jax.Array,
    gamma: jax.Array,
):
    m, n = x.shape
    assert sum(_CHUNKS) == m and n % _LANES == 0
    inv_width = 1.0 / (n * _N_DEV)
    n_chunks = len(_CHUNKS)
    n_head = n_chunks - _N_TAIL
    n_peers = _N_DEV - 1

    starts, blocks, n_lines = [], [], 0
    for c, size in enumerate(_CHUNKS):
        start = sum(_CHUNKS[:c])
        starts.append(start)
        blocks.append([])
        for r0 in range(start, start + size, _LANES):
            blocks[c].append((r0, min(_LANES, start + size - r0), n_lines))
            n_lines += 1

    def body(x_hbm, g_hbm, o_ref, x_buf, g_buf, mine, theirs, far_tail,
             x_sems, g_sem, send_sems, recv_sems):
        reads = []
        for c, size in enumerate(_CHUNKS):
            rows = pl.ds(starts[c], size)
            reads.append(
                pltpu.make_async_copy(x_hbm.at[rows], x_buf.at[rows], x_sems.at[c])
            )
            reads[c].start()
        read_g = pltpu.make_async_copy(g_hbm, g_buf, g_sem)
        read_g.start()

        me = lax.axis_index("i")
        peers = (me ^ 2, me ^ 1, me ^ 3)
        barrier = pltpu.get_barrier_semaphore()
        for peer in peers:
            pl.semaphore_signal(
                barrier, 1, device_id=(peer,), device_id_type=pl.DeviceIdType.MESH
            )

        sends = {}
        for c in range(n_chunks):
            reads[c].wait()
            for r0, rows, line in blocks[c]:
                v = x_buf[pl.ds(r0, rows), :]
                sq = v * v
                terms = [sq[:, j:j + _LANES] for j in range(0, n, _LANES)]
                while len(terms) > 1:
                    terms = terms[2:] + [terms[0] + terms[1]]
                mine[line] = _pack(jnp.sum(terms[0], axis=1, keepdims=True))
            if c == 0:
                pl.semaphore_wait(barrier, n_peers)
            lines = pl.ds(blocks[c][0][2], len(blocks[c]))
            for k, peer in enumerate(peers):
                sends[c, k] = pltpu.make_async_remote_copy(
                    src_ref=mine.at[lines],
                    dst_ref=(
                        far_tail.at[pl.ds(c - n_head, 1)]
                        if k == 0 and c >= n_head
                        else theirs.at[k, lines]
                    ),
                    send_sem=send_sems.at[c * n_peers + k],
                    recv_sem=recv_sems.at[c * n_peers + k],
                    device_id=(peer,),
                    device_id_type=pl.DeviceIdType.MESH,
                )
                sends[c, k].start()

        read_g.wait()
        o_ref[...] = x_buf[...] * g_buf[...]

        def scale(r0, rows, inv_rms):
            for j in range(0, n, _LANES):
                at = (pl.ds(r0, rows), pl.ds(j, _LANES))
                o_ref[at] = o_ref[at] * inv_rms

        near = {}
        for c in range(n_head, n_chunks):
            ((_, rows, line),) = blocks[c]
            sends[c, 1].wait_recv()
            sends[c, 2].wait_recv()
            total = mine[line] + theirs[1, line] + theirs[2, line]
            near[c] = _unpack(total * inv_width + _EPS, rows)
        for send in sends.values():
            send.wait_send()

        for c in range(n_head):
            for k in reversed(range(n_peers)):
                sends[c, k].wait_recv()
            for r0, rows, line in blocks[c]:
                total = (mine[line] + theirs[1, line]) + (
                    theirs[2, line] + theirs[0, line]
                )
                scale(r0, rows, _unpack(lax.rsqrt(total * inv_width + _EPS), rows))

        sublane = lax.broadcasted_iota(jnp.int32, _TILE, 0)
        for c in range(n_head, n_chunks):
            ((r0, rows, _),) = blocks[c]
            sends[c, 0].wait_recv()
            for i in range(0, rows, _SUBLANES):
                far = [
                    jnp.full(_TILE, far_tail[c - n_head, 0, i + s], jnp.float32)
                    for s in range(_SUBLANES)
                ]
                for bit in (1, 2, 4):
                    far = [
                        jnp.where((sublane & bit) == 0, far[s], far[s + 1])
                        for s in range(0, len(far), 2)
                    ]
                mean_sq = near[c][i:i + _SUBLANES] + far[0] * inv_width
                scale(r0 + i, _SUBLANES, lax.rsqrt(mean_sq))

    return pl.pallas_call(
        body,
        out_shape=jax.ShapeDtypeStruct((m, n), jnp.float32),
        in_specs=[
            pl.BlockSpec(memory_space=pltpu.HBM),
            pl.BlockSpec(memory_space=pltpu.HBM),
        ],
        out_specs=pl.BlockSpec(memory_space=pltpu.VMEM),
        scratch_shapes=[
            pltpu.VMEM((m, n), jnp.float32),
            pltpu.VMEM((1, n), jnp.float32),
            pltpu.VMEM((n_lines, 1, _LANES), jnp.float32),
            pltpu.VMEM((n_peers, n_lines, 1, _LANES), jnp.float32),
            pltpu.SMEM((_N_TAIL, 1, _LANES), jnp.float32),
            pltpu.SemaphoreType.DMA((n_chunks,)),
            pltpu.SemaphoreType.DMA,
            pltpu.SemaphoreType.DMA((n_chunks * n_peers,)),
            pltpu.SemaphoreType.DMA((n_chunks * n_peers,)),
        ],
        compiler_params=pltpu.CompilerParams(
            collective_id=0,
            disable_semaphore_checks=True,
        ),
    )(x, gamma.reshape(1, n))
```
